```python
import numpy as np

kernel_name = "dist_moe_cap_ep_n512_d256_e4_h512"

def setup_inputs():
    x = np.random.randn(512, 256).astype(np.float32)
    router_W = np.random.randn(256, 16).astype(np.float32) * 0.1
    scores64 = x.astype(np.float64) @ router_W.astype(np.float64)
    route_idx = np.argsort(-scores64, axis=-1)[:, :1].astype(np.int32)
    expert_W = np.random.randn(16, 256, 512).astype(np.float32) * 0.02
    return {"x": x, "router_W": router_W, "route_idx": route_idx, "expert_W": expert_W}

def reference(x, router_W, route_idx, expert_W):
    counts = np.zeros(16, dtype=np.int64)
    out = np.zeros((512, 512), dtype=np.float32)
    for i in range(512):
        e = int(route_idx[i, 0])
        if counts[e] < 25:
            out[i] = x[i] @ expert_W[e]
            counts[e] += 1
    return out
```

```python
import contextlib
import json
import os
import jax
import jax.numpy as jnp
from jax import lax
from jax.experimental import pallas as pl
from jax.experimental.pallas import tpu as pltpu

N_DEV = 4
N_TOK = 512
D = 256
H = 512
E_LOC = 4
N_EXP = N_DEV * E_LOC
CAP = 25
HALF = 13
SLOTS = 32
PROF = os.environ.get("KPROF", "0") == "1"
CFG = json.loads(os.environ.get("KCFG", "{}"))
f32, bf16, i32 = jnp.float32, jnp.bfloat16, jnp.int32
MESH = pl.DeviceIdType.MESH


def scope(name):
    return jax.named_scope(name) if PROF else contextlib.nullcontext()


Z, A, DG, B = 0, 1, 2, 3
def parse(txt):
    return [tuple(int(ch) for ch in t) for t in txt.split()]


WIDE = "002 022 102 122 202 222 302 322"
PIECES = {Z: parse(WIDE), A: parse(CFG.get("pa", WIDE)), B: parse(CFG.get("pb", WIDE)),
          DG: parse(CFG.get("pd", "002 021 031 102 122 201 211 222 301 311 321 331"))}
MAXP = max(len(v) for v in PIECES.values())
FIRST = parse(CFG.get("l0", "004"))
LOADS = {Z: parse("104 204 304"), A: parse(CFG.get("la", "102 122 202 222 302 322")),
         B: parse(CFG.get("lb", "102 122 202 222 302 322")),
         DG: parse(CFG.get("ld", "104 202 222 301 311 321 331"))}
NAME = {"z": Z, "a": A, "b": B, "d": DG}


def make_programs():
    P = {p: [] for p in range(N_DEV)}
    n = {p: len(PIECES[p]) for p in PIECES}
    via_b = CFG.get("via_b", [0, 2, 3, 4, 5])

    def by_expert(src):
        return [[c for c in range(n[src]) if PIECES[src][c][0] == j] for j in range(E_LOC)]

    p = P[Z]
    for c in range(n[Z]):
        p.append(("mm", c))
        if c == 1:
            p += [("table",), ("bar",), ("send", Z, 0, A), ("send", Z, 0, B)]
        if c >= 1:
            p += [("send", Z, c, A), ("send", Z, c, B)]
        if c % 2 and c > 1:
            p.append(("scat", Z, c - 1, c))
    p.append(("scat", Z, 0, 1))
    zorder = CFG.get("zorder", "b0 a0 b1 a1 b2 a2 b3 a3 |4 b4 a4 d1 b5 a5 b6 a6 |4 d0 a7 b7 d6 d2 d7 d3 d8 d9 d4 | d10 d5 d11")
    for tok in zorder.split():
        if tok[0] == "|":
            p.append(("drain", int(tok[1:] or 0)))
            continue
        s, c = NAME[tok[0]], int(tok[1:])
        p.append(("recv", s, c))
        if s != DG:
            p.append(("send", s, c, A + B - s))
            grp = by_expert(s)[PIECES[s][c][0]]
            if PIECES[s][c][0] == E_LOC - 1:
                p.append(("scat", s, c))
            elif c == grp[-1]:
                p.append(("scat", s, *grp))
        else:
            p.append(("scat", s, c))
    for me in (A, B):
        p = P[me]
        other = A + B - me
        p.append(("bar",))
        fwd = list(via_b) if me == B else []
        for c in range(n[me]):
            if fwd and c in CFG.get("fwd_at", [7]):
                d = fwd.pop(0)
                p += [("recv", DG, d), ("send", DG, d, Z)]
            p.append(("mm", c))
            p.append(("send", me, c, Z))
            if c == 1:
                p += [("ready",), ("send", me, 0, DG)]
            if c >= 1:
                p.append(("send", me, c, DG))
        for d in fwd:
            p += [("recv", DG, d), ("send", DG, d, Z)]
        for c in range(n[Z]):
            p.append(("recv", Z, c))
            if (c < 4) == (me == A):
                p.append(("send", Z, c, DG))
        p.append(("table",))
        for j in range(E_LOC):
            p += [("scat", me, *by_expert(me)[j]), ("scat", Z, *by_expert(Z)[j])]
        if me == A:
            order = [by_expert(other)[0], by_expert(other)[1], [c for c in via_b], by_expert(other)[2], by_expert(other)[3],
                     [c for c in range(n[DG]) if c not in via_b]]
            src = [other, other, DG, other, other, DG]
        else:
            order = [[c for c in via_b], by_expert(other)[0], by_expert(other)[1],
                     [c for c in range(n[DG]) if c not in via_b], by_expert(other)[2], by_expert(other)[3]]
            src = [DG, other, other, DG, other, other]
        for i, (s, cs) in enumerate(zip(src, order)):
            if i == len(src) - 1:
                p.append(("drain", 0))
            if s == DG:
                for c in cs:
                    if me == A or c not in via_b:
                        p.append(("recv", s, c))
                    p.append(("scat", s, c))
            else:
                p += [("recv", s, c) for c in cs] + [("scat", s, *cs)]
    p = P[DG]
    late = []
    for c in range(n[DG]):
        p.append(("mm", c))
        if c in via_b:
            p += [("send", DG, c, B)]
            p += [("send", DG, c, A)] if PIECES[DG][c][0] < 2 else []
            late += [] if PIECES[DG][c][0] < 2 else [(c, A)]
        else:
            p += [("send", DG, c, Z)]
            if c > max(via_b):
                p += [("send", DG, c, B)]
            else:
                late.insert(0, (c, B))
            late.append((c, A))
    p += [("send", DG, c, d) for c, d in late]
    p.append(("table",))
    p += [("scat", DG, *cs) for cs in by_expert(DG)]
    for j in range(E_LOC):
        for s in (A, B):
            p += [("recv", s, c) for c in by_expert(s)[j]] + [("scat", s, *by_expert(s)[j])]
    for j in (0, 2, 1, 3):
        p += [("recv", Z, c) for c in by_expert(Z)[j]] + [("scat", Z, *by_expert(Z)[j])]
    p.append(("drain", 0))
    for pos, p in P.items():
        i = p.index(("mm", CFG.get("gat", {}).get(str(pos), 2)))
        p[i:i] = [("gather", j) for j in range(CFG.get("early", 2), E_LOC)]
    return P


def pallas_dist_moe_cap_ep_n512_d256_e4_h512_kernel(x, router_W, route_idx, expert_W):
    del router_W
    progs = make_programs()

    def body(r_hbm, x_hbm, w_hbm, o_ref, r_v, xg, w_v, comm, tab_v, tab_s,
             r_sem, w_sems, g_sems, t_sem, send_sems, recv_sems, ready_sem):
        cp_r = pltpu.make_async_copy(r_hbm, r_v, r_sem)
        cp_r.start()

        def w_copy(i, load):
            j, q, nq = load
            cols = pl.ds(128 * q, 128 * nq)
            return pltpu.make_async_copy(w_hbm.at[j, :, cols], w_v.at[j, :, cols], w_sems.at[i])

        for i, l in enumerate(FIRST):
            pl.delay(1)
            w_copy(i, l).start(priority=1)
        me = lax.axis_index("i")
        bar = pltpu.get_barrier_semaphore()

        def signal(sem, dst):
            pl.semaphore_signal(sem, inc=1, device_id=(dst,), device_id_type=MESH)

        def enter(pos):
            for d in {Z: (A, B, DG), A: (DG, Z), B: (DG, Z), DG: ()}[pos]:
                signal(bar, d)
            for i, l in enumerate(LOADS[pos]):
                pl.delay(1)
                w_copy(len(FIRST) + i, l).start(priority=1)

        for pos in (A, B, DG, Z):
            pl.when(me == pos)(lambda pos=pos: enter(pos))

        for j in range(E_LOC):
            xg[pl.ds(SLOTS * j + 24, 8), :] = jnp.zeros((8, D), f32)
        o_ref[...] = jnp.zeros(o_ref.shape, f32)

        @pl.when(me == DG)
        def _():
            pl.semaphore_wait(bar, 3)
            signal(ready_sem, A)
            signal(ready_sem, B)

        def counts(n_exp):
            rows = lax.broadcasted_iota(i32, (256, 128), 0)
            cols = lax.broadcasted_iota(i32, (256, 128), 1)
            tri = ((rows <= cols) | (rows >= 128)).astype(f32).astype(bf16)
            hi = max(n_exp, 8)
            sub = lax.broadcasted_iota(i32, (hi, 128), 0)
            oh, pre = [], [jnp.zeros((hi, 128), f32)]
            for b in range(4):
                rb = (r_v[pl.ds(b, 1), :] - E_LOC * me) & (N_EXP - 1)
                oh.append((rb == (sub & (n_exp - 1))).astype(f32))
                pre.append(pre[-1] + oh[-1])
            if n_exp == 4:
                oh = [jnp.where(sub < 4, oh[b], oh[b + 1]) for b in (0, 2)]
                pre = [jnp.where(sub < 4, pre[b], pre[b + 1]) for b in (0, 2)]
            lhs = jnp.concatenate([jnp.concatenate([o, q], axis=1) for o, q in zip(oh, pre)], axis=0)
            return jnp.dot(lhs.astype(bf16), tri, preferred_element_type=f32)

        def below(cum, n_exp, e):
            s = lax.broadcasted_iota(i32, (SLOTS, 128), 0).astype(f32)
            t = None
            for b in range(4):
                u = (jnp.broadcast_to(cum[n_exp * b + e:n_exp * b + e + 1, :], (SLOTS, 128)) <= s).astype(f32)
                t = u if t is None else t + u
            return t

        with scope("route"):
            cp_r.wait()
        with scope("index"):
            cum = counts(E_LOC)
            ones = jnp.ones((128, 128), bf16)

            def tokens(j):
                t = jnp.dot(below(cum, E_LOC, j).astype(bf16), ones, preferred_element_type=f32)
                return lax.bitcast_convert_type(t + 8388608.0, i32) & (N_TOK - 1)

            idx = [tokens(0)]

        def gather(j):
            with scope(f"gather{j}"):
                for s in range(CAP):
                    pltpu.make_async_copy(x_hbm.at[pl.ds(idx[j][s, 0], 1)], xg.at[pl.ds(SLOTS * j + s, 1)],
                                          g_sems.at[j]).start()

        if CFG.get("late_idx", 1):
            gather(0)
            pl.delay(1)
            idx += [tokens(j) for j in range(1, E_LOC)]
        else:
            idx += [tokens(j) for j in range(1, E_LOC)]
            gather(0)
            pl.delay(1)
        for j in range(1, CFG.get("early", 2)):
            gather(j)

        def run(pos):
            sends = []
            state = {"tab": None, "xs": {}, "w": set(), "drained": 0}

            def rdma(src, c, dst, slot):
                rows = pl.ds(0, CAP if PIECES[src][c][2] == 2 else HALF)
                return pltpu.make_async_remote_copy(
                    comm.at[(src - pos) % N_DEV, c, rows], comm.at[(src - dst) % N_DEV, c, rows],
                    send_sems.at[slot], recv_sems.at[((src - dst) % N_DEV - 1) * MAXP + c],
                    device_id=(dst,), device_id_type=MESH)

            for op in progs[pos]:
                if op[0] == "mm":
                    c = op[1]
                    j, q, nq = PIECES[pos][c]
                    with scope(f"wait{c}"):
                        for i, (wj, wq, wn) in enumerate(FIRST + LOADS[pos]):
                            if wj == j and wq < q + nq and q < wq + wn and i not in state["w"]:
                                state["w"].add(i)
                                w_copy(i, (wj, wq, wn)).wait()
                        if j not in state["xs"]:
                            for s in range(CAP):
                                pltpu.make_async_copy(x_hbm.at[pl.ds(0, 1)], xg.at[pl.ds(SLOTS * j + s, 1)],
                                                      g_sems.at[j]).wait()
                            state["xs"][j] = xg[pl.ds(SLOTS * j, SLOTS), :].astype(bf16)
                    with scope(f"mm{c}"):
                        y = jnp.dot(state["xs"][j], w_v[j, :, pl.ds(128 * q, 128 * nq)].astype(bf16),
                                    preferred_element_type=f32)
                        y = lax.bitcast_convert_type(y.astype(bf16).astype(f32), i32)
                        if nq == 2:
                            comm[0, c] = lax.shift_right_logical(y[:, :128], 16) | y[:, 128:]
                        else:
                            comm[0, c, pl.ds(0, 16)] = lax.shift_right_logical(y[:16], 16) | y[HALF:HALF + 16]
                elif op[0] == "gather":
                    gather(op[1])
                elif op[0] == "table":
                    with scope("table"):
                        cum = counts(N_EXP)
                        allt = jnp.concatenate([below(cum, N_EXP, e) for e in range(N_EXP)], axis=0)
                        tab = lax.dot_general(jnp.ones((8, 128), bf16), allt.astype(bf16), (((1,), (1,)), ((), ())),
                                              preferred_element_type=f32)
                        slot = lax.broadcasted_iota(i32, (8, N_EXP * SLOTS), 1) & (SLOTS - 1)
                        spare = jnp.min(jnp.where(slot == CAP, tab, float(N_TOK)), axis=1, keepdims=True)
                        tok = jnp.where((tab >= N_TOK) | (slot >= CAP), spare, tab)[0:1].astype(i32)
                        tab_v[...] = ((tok >> 3) << 5) | (tok & 7)
                        state["tab"] = pltpu.make_async_copy(tab_v, tab_s, t_sem)
                        state["tab"].start()
                elif op[0] == "bar":
                    with scope("bar"):
                        pl.semaphore_wait(bar, {Z: 2, A: 1, B: 1}[pos])
                elif op[0] == "ready":
                    pl.semaphore_wait(ready_sem, 1)
                elif op[0] == "send":
                    r = rdma(op[1], op[2], op[3], len(sends))
                    r.start()
                    sends.append(r)
                elif op[0] == "recv":
                    with scope(f"recv {op[1]}.{op[2]}"):
                        rdma(op[1], op[2], pos, 0).wait_recv()
                elif op[0] == "drain":
                    with scope("drain"):
                        for r in sends[state["drained"]:max(len(sends) - op[1], 0)]:
                            r.wait_send()
                            state["drained"] += 1
                elif op[0] == "scat" and pos == Z and CFG.get("noscat"):
                    if state["tab"] is not None:
                        state["tab"].wait()
                        state["tab"] = None
                elif op[0] == "scat":
                    if state["tab"] is not None:
                        state["tab"].wait()
                        state["tab"] = None
                    k = (op[1] - pos) % N_DEV
                    j = PIECES[op[1]][op[2]][0]
                    with scope(f"scat {op[1]}.{op[2]}"):
                        for s in range(CAP):
                            t = tab_s[0, (E_LOC * k + j) * SLOTS + s]
                            for c in op[2:]:
                                _, q, nq = PIECES[op[1]][c]
                                if nq == 2:
                                    w = comm[k, c, pl.ds(s, 1), :]
                                    o_ref[pl.ds(t + 8 * q, 1), :] = lax.bitcast_convert_type(w << 16, f32)
                                    o_ref[pl.ds(t + 8 * q + 8, 1), :] = lax.bitcast_convert_type(w & (-65536), f32)
                                else:
                                    w = comm[k, c, pl.ds(s % HALF, 1), :]
                                    w = w << 16 if s < HALF else w & (-65536)
                                    o_ref[pl.ds(t + 8 * q, 1), :] = lax.bitcast_convert_type(w, f32)
            assert state["drained"] == len(sends)
            for q in range(4):
                o_ref[pl.ds(tab_s[0, CAP] + 8 * q, 1), :] = jnp.zeros((1, 128), f32)

        for pos in (DG, A, B, Z):
            pl.when(me == pos)(lambda pos=pos: run(pos))

    hbm = pl.BlockSpec(memory_space=pltpu.HBM)
    out = pl.pallas_call(
        body,
        out_shape=jax.ShapeDtypeStruct((N_TOK * H // 128, 128), f32),
        in_specs=[hbm] * 3,
        out_specs=pl.BlockSpec(memory_space=pltpu.VMEM),
        scratch_shapes=[
            pltpu.VMEM((4, 128), i32),
            pltpu.VMEM((E_LOC * SLOTS, D), f32),
            pltpu.VMEM((E_LOC, D, H), f32),
            pltpu.VMEM((N_DEV, MAXP, SLOTS, 128), i32),
            pltpu.VMEM((1, N_EXP * SLOTS), i32),
            pltpu.SMEM((1, N_EXP * SLOTS), i32),
            pltpu.SemaphoreType.DMA,
            pltpu.SemaphoreType.DMA((16,)),
            pltpu.SemaphoreType.DMA((E_LOC,)),
            pltpu.SemaphoreType.DMA,
            pltpu.SemaphoreType.DMA((4 * MAXP,)),
            pltpu.SemaphoreType.DMA((3 * MAXP,)),
            pltpu.SemaphoreType.REGULAR,
        ],
        compiler_params=pltpu.CompilerParams(collective_id=0, disable_bounds_checks=True,
                                             disable_semaphore_checks=True),
    )(route_idx.reshape(4, 128), x, expert_W)
    return out.reshape(N_TOK // 8, H // 128, 8, 128).transpose(0, 2, 1, 3).reshape(N_TOK, H)
```

```python
import jax
import jax.numpy as jnp
from jax import lax
from jax.experimental import pallas as pl
from jax.experimental.pallas import tpu as pltpu

N_DEV = 4
N_TOK = 512
D_MODEL = 256
D_OUT = 512
E_LOC = 4
N_EXP = N_DEV * E_LOC
CAP = 25
SLOTS = 32
HALF = CAP // 2
LANES = 128
SUBLANES = 8
COL_TILES = D_OUT // LANES

Z, A, D, B = 0, 1, 2, 3


def _blocks(*per_expert):
    return [(j, q, n) for j, blocks in enumerate(per_expert) for q, n in blocks]


_WHOLE = ((0, 4),)
_HALVES = ((0, 2), (2, 2))
_QUARTERS_HALF = ((0, 1), (1, 1), (2, 2))
_HALF_QUARTERS = ((0, 2), (2, 1), (3, 1))
_QUARTERS = ((1, 1), (0, 1), (3, 1), (2, 1))

W_READS = {
    Z: _blocks(_WHOLE, _WHOLE, _WHOLE, _WHOLE),
    A: _blocks(_WHOLE, _HALVES, _HALVES, _QUARTERS_HALF),
    B: _blocks(_WHOLE, _HALVES, _HALF_QUARTERS, _QUARTERS_HALF),
    D: _blocks(_WHOLE, _WHOLE, _HALVES, _QUARTERS),
}
PIECES = {
    Z: _blocks(_HALVES, _HALVES, _HALVES, _HALVES),
    A: _blocks(_HALVES, _HALVES, _HALVES, _QUARTERS_HALF),
    B: _blocks(_HALVES, _HALVES, _HALF_QUARTERS, _QUARTERS_HALF),
    D: _blocks(_QUARTERS_HALF, _HALVES, _HALF_QUARTERS, _QUARTERS),
}
MAX_READS = max(len(r) for r in W_READS.values())
MAX_PIECES = max(len(p) for p in PIECES.values())


def _ends_pair(chip, c):
    return sum(n == 1 for _, _, n in PIECES[chip][:c]) % 2 == 1


def _piece_rows(chip, c):
    if PIECES[chip][c][2] == 2:
        return CAP
    return HALF + _ends_pair(chip, c)


def _schedules():
    count = {chip: len(pieces) for chip, pieces in PIECES.items()}
    last_a, last_b = count[A] - 1, count[B] - 1
    d_via_b = [0, 2, 3, 5, 6]
    d_direct = [c for c in range(count[D]) if c not in d_via_b]

    def of_expert(chip, j):
        return [c for c, piece in enumerate(PIECES[chip]) if piece[0] == j]

    def take(chip, j):
        cs = of_expert(chip, j)
        return [("recv", chip, c) for c in cs] + [("scatter", chip, *cs)]

    z = []
    for c in range(count[Z]):
        if c == 2:
            z.append(("gather", 3))
        z.append(("matmul", c))
        if c == 1:
            z += [("entered",), ("send", Z, 0, A), ("send", Z, 0, B)]
        if c >= 1:
            z += [("send", Z, c, A), ("send", Z, c, B)]
        if c == 3:
            z.append(("table",))
    z += [("scatter", Z, *of_expert(Z, j)) for j in range(E_LOC)]
    arrivals = [
        (B, 0), (A, 0), (B, 1), (A, 1), (B, 2), (A, 2), (B, 3), (A, 3), (D, 1), (B, 4),
        (A, 4), (B, 5), (B, 6), (A, 5), (B, 7), (A, 6), (B, 8), (D, 0), (B, 9), (A, 7),
        (D, 4), (D, 2), (D, 7), (D, 8), (A, 8), (D, 9), (D, 3), (D, 10), (D, 5), (D, 6),
        (D, 11),
    ]
    for src, c in arrivals:
        if (src, c) == (B, 9):
            z.append(("flush", 8))
        if (src, c) == (A, 8):
            z.append(("flush", 0))
        z.append(("recv", src, c))
        if src != D and c < count[src] - 1:
            z.append(("send", src, c, A + B - src))
        z.append(("scatter", src, c))

    def neighbour(me):
        other = A + B - me
        p = [("entered",)]
        for c in range(count[me]):
            if c == 2:
                p.append(("gather", 3))
            if (me, c) == (B, last_b):
                p += [("recv", D, d_via_b[0]), ("send", D, d_via_b[0], Z)]
            p += [("matmul", c), ("send", me, c, Z)]
            if c == 1:
                p += [("ready",), ("send", me, 0, D)]
            if (me, c) == (A, last_a):
                p.append(("send", A, c, B))
            if c >= 1:
                p.append(("send", me, c, D))
        if me == B:
            for c in d_via_b[1:]:
                p += [("recv", D, c), ("send", D, c, Z)]
        for c in range(count[Z]):
            second_half = c >= count[Z] // 2
            if c == count[Z] // 2:
                p.append(("table",))
            p.append(("recv", Z, c))
            if second_half == (me == B):
                p.append(("send", Z, c, D))
        for j in range(E_LOC):
            p += [("scatter", me, *of_expert(me, j)), ("scatter", Z, *of_expert(Z, j))]
        for j, from_d in enumerate((d_via_b, d_direct[:3], d_direct[3:])):
            p += take(other, j)
            for c in from_d:
                if me == A or c not in d_via_b:
                    p.append(("recv", D, c))
                p.append(("scatter", D, c))
        p.append(("flush", 0))
        for c in of_expert(other, E_LOC - 1):
            p += [("recv", other, c), ("scatter", other, c)]
        return p

    d = []
    early_to_a = {2: (0, 1, 2), 4: (3,)}
    for c in range(count[D]):
        if c == 2:
            d.append(("gather", 3))
        if c != 7:
            d.append(("matmul", 6, 7) if c == 6 else ("matmul", c))
        d.append(("send", D, c, B if c in d_via_b else Z))
        if c > d_via_b[-1]:
            d.append(("send", D, c, B))
        d += [("send", D, k, A) for k in early_to_a.get(c, ())]
    d += [("send", D, c, B) for c in d_direct if c < d_via_b[-1]]
    d += [("send", D, c, A) for c in range(4, count[D])]
    d.append(("table",))
    d += [("scatter", D, *of_expert(D, j)) for j in range(E_LOC)]
    d += [("recv", B, last_b), ("send", B, last_b, A)]
    for j in range(E_LOC):
        d += take(A, j)
        d += [step for step in take(B, j) if step != ("recv", B, last_b)]
    for j in range(E_LOC):
        d += take(Z, j)
    d.append(("flush", 0))

    return {Z: z, A: neighbour(A), D: d, B: neighbour(B)}


def _keep_order():
    pl.delay(1)


def _pack(lo, hi):
    both = jnp.concatenate([lo, hi], axis=1).astype(jnp.bfloat16).astype(jnp.float32)
    bits = lax.bitcast_convert_type(both, jnp.int32)
    return lax.shift_right_logical(bits[:, :LANES], 16) | bits[:, LANES:]


def _unpack(words, half):
    bits = words & -65536 if half else words << 16
    return lax.bitcast_convert_type(bits, jnp.float32)


def _running_counts(route_ref, experts, n):
    rows = lax.broadcasted_iota(jnp.int32, (2 * LANES, LANES), 0)
    cols = lax.broadcasted_iota(jnp.int32, (2 * LANES, LANES), 1)
    summed = ((rows <= cols) | (rows >= LANES)).astype(jnp.float32)
    this, before = [], [jnp.zeros(experts.shape, jnp.float32)]
    for b in range(N_TOK // LANES):
        route = route_ref[pl.ds(b, 1), :] & (N_EXP - 1)
        this.append((route == experts).astype(jnp.float32))
        before.append(before[-1] + this[-1])
    if n < SUBLANES:
        upper = lax.broadcasted_iota(jnp.int32, experts.shape, 0) < n
        this = [jnp.where(upper, this[b], this[b + 1]) for b in (0, 2)]
        before = [jnp.where(upper, before[b], before[b + 1]) for b in (0, 2)]
    hits = jnp.concatenate(
        [jnp.concatenate([t, p], axis=1) for t, p in zip(this, before)], axis=0
    )
    return jnp.dot(hits.astype(jnp.bfloat16), summed.astype(jnp.bfloat16),
                   preferred_element_type=jnp.float32)


def _tokens_before_slot(counts, n, e):
    slot = lax.broadcasted_iota(jnp.int32, (SLOTS, LANES), 0).astype(jnp.float32)
    total = None
    for b in range(N_TOK // LANES):
        count = jnp.broadcast_to(counts[n * b + e:n * b + e + 1, :], (SLOTS, LANES))
        before = (count <= slot).astype(jnp.float32)
        total = before if total is None else total + before
    return total


def _body(route_hbm, x_hbm, w_hbm, out_ref,
          route_ref, x_rows, w_wide, w_narrow, pieces, table_vmem, table,
          route_sem, x_sems, w_sems, table_sem, send_sems, recv_sems, ready_sem):
    def read_w(i, block):
        j, q, n = block
        cols = pl.ds(LANES * q, LANES * n)
        dst = w_narrow.at[i] if n == 1 else w_wide.at[j, :, cols]
        return pltpu.make_async_copy(w_hbm.at[j, :, cols], dst, w_sems.at[i])

    def signal(sem, chip):
        pl.semaphore_signal(sem, inc=1, device_id=(chip,),
                            device_id_type=pl.DeviceIdType.MESH)

    read_route = pltpu.make_async_copy(route_hbm, route_ref, route_sem)
    read_route.start()
    _keep_order()
    read_w(0, W_READS[Z][0]).start(priority=1)

    me = lax.axis_index("i")
    barrier = pltpu.get_barrier_semaphore()
    announce_to = {Z: (A, B, D), A: (D, Z), B: (D, Z), D: ()}

    def enter(pos):
        for chip in announce_to[pos]:
            signal(barrier, chip)
        for i, block in enumerate(W_READS[pos][1:], start=1):
            _keep_order()
            read_w(i, block).start(priority=1)

    def wait_entered(pos):
        pl.semaphore_wait(barrier, sum(pos in chips for chips in announce_to.values()))

    for pos in (A, B, D, Z):
        pl.when(me == pos)(lambda pos=pos: enter(pos))

    for j in range(E_LOC):
        x_rows[pl.ds(SLOTS * (j + 1) - SUBLANES, SUBLANES), :] = jnp.zeros(
            (SUBLANES, D_MODEL), jnp.float32)
    out_ref[...] = jnp.zeros(out_ref.shape, jnp.float32)

    @pl.when(me == D)
    def _():
        wait_entered(D)
        signal(ready_sem, A)
        signal(ready_sem, B)

    local = E_LOC * me + (
        lax.broadcasted_iota(jnp.int32, (SUBLANES, LANES), 0) & (E_LOC - 1))
    read_route.wait()
    local_counts = _running_counts(route_ref, local, E_LOC)

    def slot_tokens(j):
        token = jnp.dot(_tokens_before_slot(local_counts, E_LOC, j).astype(jnp.bfloat16),
                        jnp.ones((LANES, LANES), jnp.bfloat16),
                        preferred_element_type=jnp.float32)
        return lax.bitcast_convert_type(token + 2.0**23, jnp.int32) & (N_TOK - 1)

    def gather(j, tokens):
        copies = [
            pltpu.make_async_copy(x_hbm.at[pl.ds(tokens[s, 0], 1)],
                                  x_rows.at[pl.ds(SLOTS * j + s, 1)], x_sems.at[j])
            for s in range(CAP)
        ]
        for copy in copies:
            copy.start()
        return copies

    gathers = {0: gather(0, slot_tokens(0))}
    _keep_order()
    tokens = {j: slot_tokens(j) for j in range(1, E_LOC)}
    for j in (1, 2):
        gathers[j] = gather(j, tokens[j])

    def build_table():
        every = lax.broadcasted_iota(jnp.int32, (N_EXP, LANES), 0)
        counts = _running_counts(route_ref, every, N_EXP)
        before = jnp.concatenate(
            [_tokens_before_slot(counts, N_EXP, e) for e in range(N_EXP)], axis=0)
        token = lax.dot_general(
            jnp.ones((SUBLANES, LANES), jnp.bfloat16), before.astype(jnp.bfloat16),
            (((1,), (1,)), ((), ())), preferred_element_type=jnp.float32)
        slot = lax.broadcasted_iota(jnp.int32, token.shape, 1) & (SLOTS - 1)
        spare = jnp.min(jnp.where(slot == CAP, token, float(N_TOK)), axis=1,
                        keepdims=True)
        token = jnp.where((token >= N_TOK) | (slot >= CAP), spare, token)
        token = token[0:1].astype(jnp.int32)
        table_vmem[...] = ((token >> 3) << 5) | (token & 7)
        copy = pltpu.make_async_copy(table_vmem, table, table_sem)
        copy.start()
        return copy

    def run(pos, steps):
        pending_rows = dict(gathers)
        pending_w = dict(enumerate(W_READS[pos]))
        pending_table, sends, flushed = [], [], 0
        x_of, pair_start = {}, None

        def held(src, c, by):
            return pieces.at[(src - by) % N_DEV, c, pl.ds(0, _piece_rows(src, c))]

        def remote_copy(src, c, dst):
            return pltpu.make_async_remote_copy(
                held(src, c, pos), held(src, c, dst), send_sems.at[len(sends)],
                recv_sems.at[((src - dst) % N_DEV - 1) * MAX_PIECES + c],
                device_id=(dst,), device_id_type=pl.DeviceIdType.MESH)

        for op, *args in steps:
            if op == "gather":
                (j,) = args
                pending_rows[j] = gather(j, tokens[j])
            elif op == "matmul":
                j, q, _ = PIECES[pos][args[0]]
                n = sum(PIECES[pos][c][2] for c in args)
                if j in pending_rows:
                    for copy in pending_rows.pop(j):
                        copy.wait()
                    x_of[j] = x_rows[pl.ds(SLOTS * j, SLOTS), :].astype(jnp.bfloat16)
                for i, (wj, wq, wn) in list(pending_w.items()):
                    if wj == j and wq < q + n and q < wq + wn:
                        read_w(i, pending_w.pop(i)).wait()
                if (j, q, 1) in W_READS[pos]:
                    w = w_narrow[W_READS[pos].index((j, q, 1))]
                else:
                    w = w_wide[j, :, pl.ds(LANES * q, LANES * n)]
                y = jnp.dot(x_of[j], w.astype(jnp.bfloat16),
                            preferred_element_type=jnp.float32)
                for c in args:
                    _, pq, pn = PIECES[pos][c]
                    u = y[:, LANES * (pq - q):LANES * (pq - q + pn)]
                    if pn == 2:
                        pieces[0, c] = _pack(u[:, :LANES], u[:, LANES:])
                        continue
                    lo, hi = u[:16], u[HALF:HALF + 16]
                    if _ends_pair(pos, c):
                        row = lax.broadcasted_iota(jnp.int32, lo.shape, 0)
                        lo = jnp.where(row == HALF, pair_start, lo)
                    pair_start = hi
                    pieces[0, c, pl.ds(0, 16)] = _pack(lo, hi)
            elif op == "send":
                copy = remote_copy(*args)
                copy.start()
                sends.append(copy)
            elif op == "recv":
                remote_copy(*args, pos).wait_recv()
            elif op == "table":
                pending_table.append(build_table())
            elif op == "scatter":
                src, *cs = args
                if pending_table:
                    pending_table.pop().wait()
                k = (src - pos) % N_DEV
                expert = E_LOC * src + PIECES[src][cs[0]][0]
                for s in range(CAP):
                    start = table[0, SLOTS * expert + s]
                    for c in cs:
                        _, q, n = PIECES[src][c]
                        if n == 2:
                            row, parts = s, ((q, 0), (q + 1, 1))
                        elif s < 2 * HALF:
                            row, parts = s % HALF, ((q, s // HALF),)
                        elif _ends_pair(src, c):
                            row, parts = HALF, ((PIECES[src][c - 1][1], 0), (q, 1))
                        else:
                            continue
                        words = pieces[k, c, pl.ds(row, 1), :]
                        for tile, half in parts:
                            out_ref[pl.ds(start + SUBLANES * tile, 1), :] = _unpack(
                                words, half)
            elif op == "entered":
                wait_entered(pos)
            elif op == "ready":
                pl.semaphore_wait(ready_sem, 1)
            elif op == "flush":
                while flushed < len(sends) - args[0]:
                    sends[flushed].wait_send()
                    flushed += 1
        assert flushed == len(sends) and not (pending_rows or pending_w or pending_table)

        for tile in range(COL_TILES):
            out_ref[pl.ds(table[0, CAP] + SUBLANES * tile, 1), :] = jnp.zeros(
                (1, LANES), jnp.float32)

    schedules = _schedules()
    for pos in (D, A, B, Z):
        pl.when(me == pos)(lambda pos=pos: run(pos, schedules[pos]))


def pallas_dist_moe_cap_ep_n512_d256_e4_h512_kernel(
    x: jax.Array,
    router_W: jax.Array,
    route_idx: jax.Array,
    expert_W: jax.Array,
):
    del router_W
    max_sends = max(
        sum(step[0] == "send" for step in steps) for steps in _schedules().values())
    in_hbm = pl.BlockSpec(memory_space=pltpu.HBM)
    out = pl.pallas_call(
        _body,
        out_shape=jax.ShapeDtypeStruct((N_TOK * COL_TILES, LANES), jnp.float32),
        in_specs=[in_hbm, in_hbm, in_hbm],
        out_specs=pl.BlockSpec(memory_space=pltpu.VMEM),
        scratch_shapes=[
            pltpu.VMEM((N_TOK // LANES, LANES), jnp.int32),
            pltpu.VMEM((E_LOC * SLOTS, D_MODEL), jnp.float32),
            pltpu.VMEM((E_LOC, D_MODEL, D_OUT), jnp.float32),
            pltpu.VMEM((MAX_READS, D_MODEL, LANES), jnp.float32),
            pltpu.VMEM((N_DEV, MAX_PIECES, SLOTS, LANES), jnp.int32),
            pltpu.VMEM((1, N_EXP * SLOTS), jnp.int32),
            pltpu.SMEM((1, N_EXP * SLOTS), jnp.int32),
            pltpu.SemaphoreType.DMA,
            pltpu.SemaphoreType.DMA((E_LOC,)),
            pltpu.SemaphoreType.DMA((MAX_READS,)),
            pltpu.SemaphoreType.DMA,
            pltpu.SemaphoreType.DMA((max_sends + 1,)),
            pltpu.SemaphoreType.DMA(((N_DEV - 1) * MAX_PIECES,)),
            pltpu.SemaphoreType.REGULAR,
        ],
        compiler_params=pltpu.CompilerParams(
            collective_id=0, disable_bounds_checks=True, disable_semaphore_checks=True),
    )(route_idx.reshape(N_TOK // LANES, LANES), x, expert_W)
    out = out.reshape(N_TOK // SUBLANES, COL_TILES, SUBLANES, LANES)
    return out.transpose(0, 2, 1, 3).reshape(N_TOK, D_OUT)
```

```python
import jax
import jax.numpy as jnp
from jax import lax
from jax.experimental import pallas as pl
from jax.experimental.pallas import tpu as pltpu

N_DEV = 4
N_TOK = 512
D_MODEL = 256
D_OUT = 512
E_LOC = 4
N_EXP = N_DEV * E_LOC
CAP = 25
SLOTS = 32
HALF = CAP // 2
LANES = 128
SUBLANES = 8
COL_TILES = D_OUT // LANES

Z, A, D, B = 0, 1, 2, 3


def _blocks(*per_expert):
    return [(j, q, n) for j, blocks in enumerate(per_expert) for q, n in blocks]


_WHOLE = ((0, 4),)
_HALVES = ((0, 2), (2, 2))
_QUARTERS_HALF = ((1, 1), (0, 1), (2, 2))
_HALF_QUARTERS = ((0, 2), (3, 1), (2, 1))
_QUARTERS = ((1, 1), (0, 1), (3, 1), (2, 1))

W_READS = {
    Z: _blocks(_WHOLE, _WHOLE, _WHOLE, _WHOLE),
    A: _blocks(_WHOLE, _HALVES, _HALVES, _QUARTERS_HALF),
    B: _blocks(_WHOLE, _HALVES, _HALF_QUARTERS, _QUARTERS_HALF),
    D: _blocks(_WHOLE, _WHOLE, _HALVES, _QUARTERS),
}
PIECES = {
    Z: _blocks(_HALVES, _HALVES, _HALVES, _HALVES),
    A: _blocks(_HALVES, _HALVES, _HALVES, _QUARTERS_HALF),
    B: _blocks(_HALVES, _HALVES, _HALF_QUARTERS, _QUARTERS_HALF),
    D: _blocks(_QUARTERS_HALF, _HALVES, _HALF_QUARTERS, _QUARTERS),
}
MAX_READS = max(len(r) for r in W_READS.values())
MAX_PIECES = max(len(p) for p in PIECES.values())


def _ends_pair(chip, c):
    return sum(n == 1 for _, _, n in PIECES[chip][:c]) % 2 == 1


def _piece_rows(chip, c):
    if PIECES[chip][c][2] == 2:
        return CAP
    return HALF + _ends_pair(chip, c)


def _schedules():
    count = {chip: len(pieces) for chip, pieces in PIECES.items()}
    last_a, last_b = count[A] - 1, count[B] - 1
    d_via_b = [0, 2, 3, 5, 6]
    d_direct = [c for c in range(count[D]) if c not in d_via_b]

    def of_expert(chip, j):
        return [c for c, piece in enumerate(PIECES[chip]) if piece[0] == j]

    def take(chip, j):
        cs = of_expert(chip, j)
        return [("recv", chip, c) for c in cs] + [("scatter", chip, *cs)]

    z = []
    for c in range(count[Z]):
        z.append(("matmul", c))
        if c == 1:
            z += [("entered",), ("send", Z, 0, A), ("send", Z, 0, B)]
        if c >= 1:
            z += [("send", Z, c, A), ("send", Z, c, B)]
        if c == 3:
            z.append(("table",))
    z += [("scatter", Z, *of_expert(Z, j)) for j in range(E_LOC)]
    arrivals = [
        (B, 0), (A, 0), (B, 1), (A, 1), (B, 2), (A, 2), (B, 3), (A, 3), (D, 1), (B, 4),
        (A, 4), (B, 5), (B, 6), (A, 5), (B, 7), (A, 6), (B, 8), (D, 0), (B, 9), (A, 7),
        (D, 4), (D, 2), (D, 7), (D, 8), (A, 8), (D, 9), (D, 3), (D, 10), (D, 5), (D, 6),
        (D, 11),
    ]
    for src, c in arrivals:
        if (src, c) == (B, 9):
            z.append(("flush", 8))
        if (src, c) == (A, 8):
            z.append(("flush", 0))
        z.append(("recv", src, c))
        if src != D and c < count[src] - 1:
            z.append(("send", src, c, A + B - src))
        z.append(("scatter", src, c))

    def neighbour(me):
        other = A + B - me
        p = [("entered",)]
        for c in range(count[me]):
            if (me, c) == (B, last_b):
                p += [("recv", D, d_via_b[0]), ("send", D, d_via_b[0], Z)]
            p += [("matmul", c), ("send", me, c, Z)]
            if c == 1:
                p += [("ready",), ("send", me, 0, D)]
            if (me, c) == (A, last_a):
                p.append(("send", A, c, B))
            if c >= 1:
                p.append(("send", me, c, D))
        if me == B:
            for c in d_via_b[1:]:
                p += [("recv", D, c), ("send", D, c, Z)]
        for c in range(count[Z]):
            second_half = c >= count[Z] // 2
            if c == count[Z] // 2:
                p.append(("table",))
            p.append(("recv", Z, c))
            if second_half == (me == B):
                p.append(("send", Z, c, D))
        for j in range(E_LOC):
            p += [("scatter", me, *of_expert(me, j)), ("scatter", Z, *of_expert(Z, j))]
        for j, from_d in enumerate((d_via_b, d_direct[:3], d_direct[3:])):
            p += take(other, j)
            for c in from_d:
                if me == A or c not in d_via_b:
                    p.append(("recv", D, c))
                p.append(("scatter", D, c))
        p.append(("flush", 0))
        for c in of_expert(other, E_LOC - 1):
            p += [("recv", other, c), ("scatter", other, c)]
        return p

    d = []
    early_to_a = {2: (0, 1, 2), 4: (3,)}
    for c in range(count[D]):
        if c != 7:
            d.append(("matmul", 6, 7) if c == 6 else ("matmul", c))
        d.append(("send", D, c, B if c in d_via_b else Z))
        if c > d_via_b[-1]:
            d.append(("send", D, c, B))
        d += [("send", D, k, A) for k in early_to_a.get(c, ())]
    d += [("send", D, c, B) for c in d_direct if c < d_via_b[-1]]
    d += [("send", D, c, A) for c in range(4, count[D])]
    d.append(("table",))
    d += [("scatter", D, *of_expert(D, j)) for j in range(E_LOC)]
    d += [("recv", B, last_b), ("send", B, last_b, A)]
    for j in range(E_LOC):
        d += take(A, j)
        d += [step for step in take(B, j) if step != ("recv", B, last_b)]
    for j in range(E_LOC):
        d += take(Z, j)
    d.append(("flush", 0))

    return {Z: z, A: neighbour(A), D: d, B: neighbour(B)}


def _keep_order():
    pl.delay(1)


def _pack(lo, hi):
    both = jnp.concatenate([lo, hi], axis=1).astype(jnp.bfloat16).astype(jnp.float32)
    bits = lax.bitcast_convert_type(both, jnp.int32)
    return lax.shift_right_logical(bits[:, :LANES], 16) | bits[:, LANES:]


def _unpack(words, half):
    bits = words & -65536 if half else words << 16
    return lax.bitcast_convert_type(bits, jnp.float32)


def _running_counts(route_ref, experts, n):
    rows = lax.broadcasted_iota(jnp.int32, (2 * LANES, LANES), 0)
    cols = lax.broadcasted_iota(jnp.int32, (2 * LANES, LANES), 1)
    summed = ((rows <= cols) | (rows >= LANES)).astype(jnp.float32)
    this, before = [], [jnp.zeros(experts.shape, jnp.float32)]
    for b in range(N_TOK // LANES):
        route = route_ref[pl.ds(b, 1), :] & (N_EXP - 1)
        this.append((route == experts).astype(jnp.float32))
        before.append(before[-1] + this[-1])
    if n < SUBLANES:
        upper = lax.broadcasted_iota(jnp.int32, experts.shape, 0) < n
        this = [jnp.where(upper, this[b], this[b + 1]) for b in (0, 2)]
        before = [jnp.where(upper, before[b], before[b + 1]) for b in (0, 2)]
    hits = jnp.concatenate(
        [jnp.concatenate([t, p], axis=1) for t, p in zip(this, before)], axis=0
    )
    return jnp.dot(hits.astype(jnp.bfloat16), summed.astype(jnp.bfloat16),
                   preferred_element_type=jnp.float32)


def _tokens_before_slot(counts, n, e):
    slot = lax.broadcasted_iota(jnp.int32, (SLOTS, LANES), 0).astype(jnp.float32)
    total = None
    for b in range(N_TOK // LANES):
        count = jnp.broadcast_to(counts[n * b + e:n * b + e + 1, :], (SLOTS, LANES))
        before = (count <= slot).astype(jnp.float32)
        total = before if total is None else total + before
    return total


def _body(route_hbm, x_hbm, w_hbm, out_ref,
          route_ref, x_rows, w_wide, w_narrow, pieces, table_vmem, table,
          route_sem, x_sems, w_sems, table_sem, send_sems, recv_sems, ready_sem):
    def read_w(i, block):
        j, q, n = block
        cols = pl.ds(LANES * q, LANES * n)
        dst = w_narrow.at[i] if n == 1 else w_wide.at[j, :, cols]
        return pltpu.make_async_copy(w_hbm.at[j, :, cols], dst, w_sems.at[i])

    def signal(sem, chip):
        pl.semaphore_signal(sem, inc=1, device_id=(chip,),
                            device_id_type=pl.DeviceIdType.MESH)

    read_route = pltpu.make_async_copy(route_hbm, route_ref, route_sem)
    read_route.start()
    _keep_order()
    read_w(0, W_READS[Z][0]).start(priority=1)

    me = lax.axis_index("i")
    barrier = pltpu.get_barrier_semaphore()
    announce_to = {Z: (A, B, D), A: (D, Z), B: (D, Z), D: ()}

    def enter(pos):
        for chip in announce_to[pos]:
            signal(barrier, chip)
        for i, block in enumerate(W_READS[pos][1:], start=1):
            _keep_order()
            read_w(i, block).start(priority=1)

    def wait_entered(pos):
        pl.semaphore_wait(barrier, sum(pos in chips for chips in announce_to.values()))

    for pos in (A, B, D, Z):
        pl.when(me == pos)(lambda pos=pos: enter(pos))

    for j in range(E_LOC):
        x_rows[pl.ds(SLOTS * (j + 1) - SUBLANES, SUBLANES), :] = jnp.zeros(
            (SUBLANES, D_MODEL), jnp.float32)
    out_ref[...] = jnp.zeros(out_ref.shape, jnp.float32)

    @pl.when(me == D)
    def _():
        wait_entered(D)
        signal(ready_sem, A)
        signal(ready_sem, B)

    local = E_LOC * me + (
        lax.broadcasted_iota(jnp.int32, (SUBLANES, LANES), 0) & (E_LOC - 1))
    read_route.wait()
    local_counts = _running_counts(route_ref, local, E_LOC)

    def gather(j):
        token = jnp.dot(_tokens_before_slot(local_counts, E_LOC, j).astype(jnp.bfloat16),
                        jnp.ones((LANES, LANES), jnp.bfloat16),
                        preferred_element_type=jnp.float32)
        token = lax.bitcast_convert_type(token + 2.0**23, jnp.int32) & (N_TOK - 1)
        copies = [
            pltpu.make_async_copy(x_hbm.at[pl.ds(token[s, 0], 1)],
                                  x_rows.at[pl.ds(SLOTS * j + s, 1)], x_sems.at[j])
            for s in range(CAP)
        ]
        for copy in copies:
            copy.start()
        return copies

    gathers = [gather(0)]
    _keep_order()
    gathers += [gather(j) for j in range(1, E_LOC)]

    def build_table():
        every = lax.broadcasted_iota(jnp.int32, (N_EXP, LANES), 0)
        counts = _running_counts(route_ref, every, N_EXP)
        before = jnp.concatenate(
            [_tokens_before_slot(counts, N_EXP, e) for e in range(N_EXP)], axis=0)
        token = lax.dot_general(
            jnp.ones((SUBLANES, LANES), jnp.bfloat16), before.astype(jnp.bfloat16),
            (((1,), (1,)), ((), ())), preferred_element_type=jnp.float32)
        slot = lax.broadcasted_iota(jnp.int32, token.shape, 1) & (SLOTS - 1)
        spare = jnp.min(jnp.where(slot == CAP, token, float(N_TOK)), axis=1,
                        keepdims=True)
        token = jnp.where((token >= N_TOK) | (slot >= CAP), spare, token)
        token = token[0:1].astype(jnp.int32)
        table_vmem[...] = ((token >> 3) << 5) | (token & 7)
        copy = pltpu.make_async_copy(table_vmem, table, table_sem)
        copy.start()
        return copy

    def run(pos, steps):
        pending_rows = dict(enumerate(gathers))
        pending_w = dict(enumerate(W_READS[pos]))
        pending_table, sends, flushed = [], [], 0
        x_of, pair_start = {}, None

        def held(src, c, by):
            return pieces.at[(src - by) % N_DEV, c, pl.ds(0, _piece_rows(src, c))]

        def remote_copy(src, c, dst):
            return pltpu.make_async_remote_copy(
                held(src, c, pos), held(src, c, dst), send_sems.at[len(sends)],
                recv_sems.at[((src - dst) % N_DEV - 1) * MAX_PIECES + c],
                device_id=(dst,), device_id_type=pl.DeviceIdType.MESH)

        for op, *args in steps:
            if op == "matmul":
                j, q, _ = min(PIECES[pos][c] for c in args)
                n = sum(PIECES[pos][c][2] for c in args)
                if j in pending_rows:
                    for copy in pending_rows.pop(j):
                        copy.wait()
                    x_of[j] = x_rows[pl.ds(SLOTS * j, SLOTS), :].astype(jnp.bfloat16)
                for i, (wj, wq, wn) in list(pending_w.items()):
                    if wj == j and wq < q + n and q < wq + wn:
                        read_w(i, pending_w.pop(i)).wait()
                if (j, q, 1) in W_READS[pos]:
                    w = w_narrow[W_READS[pos].index((j, q, 1))]
                else:
                    w = w_wide[j, :, pl.ds(LANES * q, LANES * n)]
                y = jnp.dot(x_of[j], w.astype(jnp.bfloat16),
                            preferred_element_type=jnp.float32)
                for c in args:
                    _, pq, pn = PIECES[pos][c]
                    u = y[:, LANES * (pq - q):LANES * (pq - q + pn)]
                    if pn == 2:
                        pieces[0, c] = _pack(u[:, :LANES], u[:, LANES:])
                        continue
                    lo, hi = u[:16], u[HALF:HALF + 16]
                    if _ends_pair(pos, c):
                        row = lax.broadcasted_iota(jnp.int32, lo.shape, 0)
                        lo = jnp.where(row == HALF, pair_start, lo)
                    pair_start = hi
                    pieces[0, c, pl.ds(0, 16)] = _pack(lo, hi)
            elif op == "send":
                copy = remote_copy(*args)
                copy.start()
                sends.append(copy)
            elif op == "recv":
                remote_copy(*args, pos).wait_recv()
            elif op == "table":
                pending_table.append(build_table())
            elif op == "scatter":
                src, *cs = args
                if pending_table:
                    pending_table.pop().wait()
                k = (src - pos) % N_DEV
                expert = E_LOC * src + PIECES[src][cs[0]][0]
                for s in range(CAP):
                    start = table[0, SLOTS * expert + s]
                    for c in cs:
                        _, q, n = PIECES[src][c]
                        if n == 2:
                            row, parts = s, ((q, 0), (q + 1, 1))
                        elif s < 2 * HALF:
                            row, parts = s % HALF, ((q, s // HALF),)
                        elif _ends_pair(src, c):
                            row, parts = HALF, ((PIECES[src][c - 1][1], 0), (q, 1))
                        else:
                            continue
                        words = pieces[k, c, pl.ds(row, 1), :]
                        for tile, half in parts:
                            out_ref[pl.ds(start + SUBLANES * tile, 1), :] = _unpack(
                                words, half)
            elif op == "entered":
                wait_entered(pos)
            elif op == "ready":
                pl.semaphore_wait(ready_sem, 1)
            elif op == "flush":
                while flushed < len(sends) - args[0]:
                    sends[flushed].wait_send()
                    flushed += 1
        assert flushed == len(sends) and not (pending_rows or pending_w or pending_table)

        for tile in range(COL_TILES):
            out_ref[pl.ds(table[0, CAP] + SUBLANES * tile, 1), :] = jnp.zeros(
                (1, LANES), jnp.float32)

    schedules = _schedules()
    for pos in (D, A, B, Z):
        pl.when(me == pos)(lambda pos=pos: run(pos, schedules[pos]))


def pallas_dist_moe_cap_ep_n512_d256_e4_h512_kernel(
    x: jax.Array,
    router_W: jax.Array,
    route_idx: jax.Array,
    expert_W: jax.Array,
):
    del router_W
    max_sends = max(
        sum(step[0] == "send" for step in steps) for steps in _schedules().values())
    in_hbm = pl.BlockSpec(memory_space=pltpu.HBM)
    out = pl.pallas_call(
        _body,
        out_shape=jax.ShapeDtypeStruct((N_TOK * COL_TILES, LANES), jnp.float32),
        in_specs=[in_hbm, in_hbm, in_hbm],
        out_specs=pl.BlockSpec(memory_space=pltpu.VMEM),
        scratch_shapes=[
            pltpu.VMEM((N_TOK // LANES, LANES), jnp.int32),
            pltpu.VMEM((E_LOC * SLOTS, D_MODEL), jnp.float32),
            pltpu.VMEM((E_LOC, D_MODEL, D_OUT), jnp.float32),
            pltpu.VMEM((MAX_READS, D_MODEL, LANES), jnp.float32),
            pltpu.VMEM((N_DEV, MAX_PIECES, SLOTS, LANES), jnp.int32),
            pltpu.VMEM((1, N_EXP * SLOTS), jnp.int32),
            pltpu.SMEM((1, N_EXP * SLOTS), jnp.int32),
            pltpu.SemaphoreType.DMA,
            pltpu.SemaphoreType.DMA((E_LOC,)),
            pltpu.SemaphoreType.DMA((MAX_READS,)),
            pltpu.SemaphoreType.DMA,
            pltpu.SemaphoreType.DMA((max_sends + 1,)),
            pltpu.SemaphoreType.DMA(((N_DEV - 1) * MAX_PIECES,)),
            pltpu.SemaphoreType.REGULAR,
        ],
        compiler_params=pltpu.CompilerParams(
            collective_id=0,
            disable_bounds_checks=True,
            disable_semaphore_checks=True,
            flags={"XLA_TPU_FORCE_LP_LLO_SCHEDULER": True},
        ),
    )(route_idx.reshape(N_TOK // LANES, LANES), x, expert_W)
    out = out.reshape(N_TOK // SUBLANES, COL_TILES, SUBLANES, LANES)
    return out.transpose(0, 2, 1, 3).reshape(N_TOK, D_OUT)
```

```python
import jax
import jax.numpy as jnp
from jax import lax
from jax.experimental import pallas as pl
from jax.experimental.pallas import tpu as pltpu

N_DEV = 4
N_TOK = 512
D_MODEL = 256
D_OUT = 512
E_LOC = 4
N_EXP = N_DEV * E_LOC
CAP = 25
SLOTS = 32
HALF = CAP // 2
LANES = 128
SUBLANES = 8
COL_TILES = D_OUT // LANES

Z, A, D, B = 0, 1, 2, 3


def _blocks(*per_expert):
    return [(j, q, n) for j, blocks in enumerate(per_expert) for q, n in blocks]


_WHOLE = ((0, 4),)
_HALVES = ((0, 2), (2, 2))
_QUARTERS_HALF = ((1, 1), (0, 1), (2, 2))
_HALF_QUARTERS = ((0, 2), (3, 1), (2, 1))
_QUARTERS = ((1, 1), (0, 1), (3, 1), (2, 1))

W_READS = {
    Z: _blocks(_WHOLE, _WHOLE, _WHOLE, _WHOLE),
    A: _blocks(_WHOLE, _HALVES, _HALVES, _QUARTERS),
    B: _blocks(_WHOLE, _HALVES, _HALF_QUARTERS, _QUARTERS),
    D: _blocks(_WHOLE, _WHOLE, _HALVES, _QUARTERS),
}
PIECES = {
    Z: _blocks(_HALVES, _HALVES, _HALVES, _HALVES),
    A: _blocks(_HALVES, _HALVES, _HALVES, _QUARTERS),
    B: _blocks(_HALVES, _HALVES, _HALF_QUARTERS, _QUARTERS),
    D: _blocks(_QUARTERS_HALF, _HALVES, _HALF_QUARTERS, _QUARTERS),
}
MAX_READS = max(len(r) for r in W_READS.values())
MAX_PIECES = max(len(p) for p in PIECES.values())


def _ends_pair(chip, c):
    return sum(n == 1 for _, _, n in PIECES[chip][:c]) % 2 == 1


def _piece_rows(chip, c):
    if PIECES[chip][c][2] == 2:
        return CAP
    return HALF + _ends_pair(chip, c)


def _schedules():
    count = {chip: len(pieces) for chip, pieces in PIECES.items()}
    last_a, last_b = count[A] - 1, count[B] - 1
    d_via_b = [0, 2, 3, 5, 6]
    d_direct = [c for c in range(count[D]) if c not in d_via_b]

    def of_expert(chip, j):
        return [c for c, piece in enumerate(PIECES[chip]) if piece[0] == j]

    def take(chip, j):
        cs = of_expert(chip, j)
        return [("recv", chip, c) for c in cs] + [("scatter", chip, *cs)]

    z = []
    for c in range(count[Z]):
        z.append(("matmul", c))
        if c == 1:
            z += [("entered",), ("send", Z, 0, A), ("send", Z, 0, B)]
        if c >= 1:
            z += [("send", Z, c, A), ("send", Z, c, B)]
        if c == 3:
            z.append(("table",))
    z += [("scatter", Z, *of_expert(Z, j)) for j in range(E_LOC)]
    arrivals = [
        (B, 0), (A, 0), (B, 1), (A, 1), (B, 2), (A, 2), (B, 3), (A, 3), (D, 1), (B, 4),
        (A, 4), (B, 5), (B, 6), (A, 5), (B, 7), (A, 6), (B, 8), (D, 0), (B, 9), (A, 7),
        (B, 10), (D, 4), (A, 8), (D, 2), (D, 7), (D, 8), (A, 9), (D, 9), (D, 3), (D, 10),
        (D, 5), (D, 6), (D, 11),
    ]
    for src, c in arrivals:
        if (src, c) == (B, last_b):
            z.append(("flush", 8))
        if (src, c) == (A, last_a):
            z.append(("flush", 0))
        z.append(("recv", src, c))
        if src != D and c < count[src] - 1:
            z.append(("send", src, c, A + B - src))
        z.append(("scatter", src, c))

    def neighbour(me):
        other = A + B - me
        p = [("entered",)]
        for c in range(count[me]):
            if (me, c) == (B, last_b - 1):
                p += [("recv", D, d_via_b[0]), ("send", D, d_via_b[0], Z)]
            p += [("matmul", c), ("send", me, c, Z)]
            if c == 1:
                p += [("ready",), ("send", me, 0, D)]
            if (me, c) == (A, last_a):
                p.append(("send", A, c, B))
            if c >= 1:
                p.append(("send", me, c, D))
        if me == B:
            for c in d_via_b[1:]:
                p += [("recv", D, c), ("send", D, c, Z)]
        for c in range(count[Z]):
            second_half = c >= count[Z] // 2
            if c == count[Z] // 2:
                p.append(("table",))
            p.append(("recv", Z, c))
            if second_half == (me == B):
                p.append(("send", Z, c, D))
        for j in range(E_LOC):
            p += [("scatter", me, *of_expert(me, j)), ("scatter", Z, *of_expert(Z, j))]
        for j, from_d in enumerate((d_via_b, d_direct[:3], d_direct[3:])):
            p += take(other, j)
            for c in from_d:
                if me == A or c not in d_via_b:
                    p.append(("recv", D, c))
                p.append(("scatter", D, c))
        p.append(("flush", 0))
        for c in of_expert(other, E_LOC - 1):
            p += [("recv", other, c), ("scatter", other, c)]
        return p

    d = []
    early_to_a = {2: (0, 1, 2), 4: (3,)}
    for c in range(count[D]):
        if c != 7:
            d.append(("matmul", 6, 7) if c == 6 else ("matmul", c))
        d.append(("send", D, c, B if c in d_via_b else Z))
        if c > d_via_b[-1]:
            d.append(("send", D, c, B))
        d += [("send", D, k, A) for k in early_to_a.get(c, ())]
    d += [("send", D, c, B) for c in d_direct if c < d_via_b[-1]]
    d += [("send", D, c, A) for c in range(4, count[D])]
    d.append(("table",))
    d += [("scatter", D, *of_expert(D, j)) for j in range(E_LOC)]
    d += [("recv", B, last_b), ("send", B, last_b, A)]
    for j in range(E_LOC):
        d += take(A, j)
        d += [step for step in take(B, j) if step != ("recv", B, last_b)]
    for j in range(E_LOC):
        d += take(Z, j)
    d.append(("flush", 0))

    return {Z: z, A: neighbour(A), D: d, B: neighbour(B)}


def _keep_order():
    pl.delay(1)


def _pack(lo, hi):
    both = jnp.concatenate([lo, hi], axis=1).astype(jnp.bfloat16).astype(jnp.float32)
    bits = lax.bitcast_convert_type(both, jnp.int32)
    return lax.shift_right_logical(bits[:, :LANES], 16) | bits[:, LANES:]


def _unpack(words, half):
    bits = words & -65536 if half else words << 16
    return lax.bitcast_convert_type(bits, jnp.float32)


def _running_counts(route_ref, experts, n):
    rows = lax.broadcasted_iota(jnp.int32, (2 * LANES, LANES), 0)
    cols = lax.broadcasted_iota(jnp.int32, (2 * LANES, LANES), 1)
    summed = ((rows <= cols) | (rows >= LANES)).astype(jnp.float32)
    this, before = [], [jnp.zeros(experts.shape, jnp.float32)]
    for b in range(N_TOK // LANES):
        route = route_ref[pl.ds(b, 1), :] & (N_EXP - 1)
        this.append((route == experts).astype(jnp.float32))
        before.append(before[-1] + this[-1])
    if n < SUBLANES:
        upper = lax.broadcasted_iota(jnp.int32, experts.shape, 0) < n
        this = [jnp.where(upper, this[b], this[b + 1]) for b in (0, 2)]
        before = [jnp.where(upper, before[b], before[b + 1]) for b in (0, 2)]
    hits = jnp.concatenate(
        [jnp.concatenate([t, p], axis=1) for t, p in zip(this, before)], axis=0
    )
    return jnp.dot(hits.astype(jnp.bfloat16), summed.astype(jnp.bfloat16),
                   preferred_element_type=jnp.float32)


def _tokens_before_slot(counts, n, e):
    slot = lax.broadcasted_iota(jnp.int32, (SLOTS, LANES), 0).astype(jnp.float32)
    total = None
    for b in range(N_TOK // LANES):
        count = jnp.broadcast_to(counts[n * b + e:n * b + e + 1, :], (SLOTS, LANES))
        before = (count <= slot).astype(jnp.float32)
        total = before if total is None else total + before
    return total


def _body(route_hbm, x_hbm, w_hbm, out_ref,
          route_ref, x_rows, w_wide, w_narrow, pieces, table_vmem, table,
          route_sem, x_sems, w_sems, table_sem, send_sems, recv_sems, ready_sem):
    def read_w(i, block):
        j, q, n = block
        cols = pl.ds(LANES * q, LANES * n)
        dst = w_narrow.at[i] if n == 1 else w_wide.at[j, :, cols]
        return pltpu.make_async_copy(w_hbm.at[j, :, cols], dst, w_sems.at[i])

    def signal(sem, chip):
        pl.semaphore_signal(sem, inc=1, device_id=(chip,),
                            device_id_type=pl.DeviceIdType.MESH)

    read_route = pltpu.make_async_copy(route_hbm, route_ref, route_sem)
    read_route.start()
    _keep_order()
    read_w(0, W_READS[Z][0]).start(priority=1)

    me = lax.axis_index("i")
    barrier = pltpu.get_barrier_semaphore()
    announce_to = {Z: (A, B, D), A: (D, Z), B: (D, Z), D: ()}

    def enter(pos):
        for chip in announce_to[pos]:
            signal(barrier, chip)
        for i, block in enumerate(W_READS[pos][1:], start=1):
            _keep_order()
            read_w(i, block).start(priority=1)

    def wait_entered(pos):
        pl.semaphore_wait(barrier, sum(pos in chips for chips in announce_to.values()))

    for pos in (A, B, D, Z):
        pl.when(me == pos)(lambda pos=pos: enter(pos))

    for j in range(E_LOC):
        x_rows[pl.ds(SLOTS * (j + 1) - SUBLANES, SUBLANES), :] = jnp.zeros(
            (SUBLANES, D_MODEL), jnp.float32)
    out_ref[...] = jnp.zeros(out_ref.shape, jnp.float32)

    @pl.when(me == D)
    def _():
        wait_entered(D)
        signal(ready_sem, A)
        signal(ready_sem, B)

    local = E_LOC * me + (
        lax.broadcasted_iota(jnp.int32, (SUBLANES, LANES), 0) & (E_LOC - 1))
    read_route.wait()
    local_counts = _running_counts(route_ref, local, E_LOC)

    def gather(j):
        token = jnp.dot(_tokens_before_slot(local_counts, E_LOC, j).astype(jnp.bfloat16),
                        jnp.ones((LANES, LANES), jnp.bfloat16),
                        preferred_element_type=jnp.float32)
        token = lax.bitcast_convert_type(token + 2.0**23, jnp.int32) & (N_TOK - 1)
        copies = [
            pltpu.make_async_copy(x_hbm.at[pl.ds(token[s, 0], 1)],
                                  x_rows.at[pl.ds(SLOTS * j + s, 1)], x_sems.at[j])
            for s in range(CAP)
        ]
        for copy in copies:
            copy.start()
        return copies

    gathers = [gather(0)]
    _keep_order()
    gathers += [gather(j) for j in range(1, E_LOC)]

    def build_table():
        every = lax.broadcasted_iota(jnp.int32, (N_EXP, LANES), 0)
        counts = _running_counts(route_ref, every, N_EXP)
        before = jnp.concatenate(
            [_tokens_before_slot(counts, N_EXP, e) for e in range(N_EXP)], axis=0)
        token = lax.dot_general(
            jnp.ones((SUBLANES, LANES), jnp.bfloat16), before.astype(jnp.bfloat16),
            (((1,), (1,)), ((), ())), preferred_element_type=jnp.float32)
        slot = lax.broadcasted_iota(jnp.int32, token.shape, 1) & (SLOTS - 1)
        spare = jnp.min(jnp.where(slot == CAP, token, float(N_TOK)), axis=1,
                        keepdims=True)
        token = jnp.where((token >= N_TOK) | (slot >= CAP), spare, token)
        token = token[0:1].astype(jnp.int32)
        table_vmem[...] = ((token >> 3) << 5) | (token & 7)
        copy = pltpu.make_async_copy(table_vmem, table, table_sem)
        copy.start()
        return copy

    def run(pos, steps):
        pending_rows = dict(enumerate(gathers))
        pending_w = dict(enumerate(W_READS[pos]))
        pending_table, sends, flushed = [], [], 0
        x_of, pair_start = {}, None

        def held(src, c, by):
            return pieces.at[(src - by) % N_DEV, c, pl.ds(0, _piece_rows(src, c))]

        def remote_copy(src, c, dst):
            return pltpu.make_async_remote_copy(
                held(src, c, pos), held(src, c, dst), send_sems.at[len(sends)],
                recv_sems.at[((src - dst) % N_DEV - 1) * MAX_PIECES + c],
                device_id=(dst,), device_id_type=pl.DeviceIdType.MESH)

        for op, *args in steps:
            if op == "matmul":
                j, q, _ = min(PIECES[pos][c] for c in args)
                n = sum(PIECES[pos][c][2] for c in args)
                if j in pending_rows:
                    for copy in pending_rows.pop(j):
                        copy.wait()
                    x_of[j] = x_rows[pl.ds(SLOTS * j, SLOTS), :].astype(jnp.bfloat16)
                for i, (wj, wq, wn) in list(pending_w.items()):
                    if wj == j and wq < q + n and q < wq + wn:
                        read_w(i, pending_w.pop(i)).wait()
                if (j, q, 1) in W_READS[pos]:
                    w = w_narrow[W_READS[pos].index((j, q, 1))]
                else:
                    w = w_wide[j, :, pl.ds(LANES * q, LANES * n)]
                y = jnp.dot(x_of[j], w.astype(jnp.bfloat16),
                            preferred_element_type=jnp.float32)
                for c in args:
                    _, pq, pn = PIECES[pos][c]
                    u = y[:, LANES * (pq - q):LANES * (pq - q + pn)]
                    if pn == 2:
                        pieces[0, c] = _pack(u[:, :LANES], u[:, LANES:])
                        continue
                    lo, hi = u[:16], u[HALF:HALF + 16]
                    if _ends_pair(pos, c):
                        row = lax.broadcasted_iota(jnp.int32, lo.shape, 0)
                        lo = jnp.where(row == HALF, pair_start, lo)
                    pair_start = hi
                    pieces[0, c, pl.ds(0, 16)] = _pack(lo, hi)
            elif op == "send":
                copy = remote_copy(*args)
                copy.start()
                sends.append(copy)
            elif op == "recv":
                remote_copy(*args, pos).wait_recv()
            elif op == "table":
                pending_table.append(build_table())
            elif op == "scatter":
                src, *cs = args
                if pending_table:
                    pending_table.pop().wait()
                k = (src - pos) % N_DEV
                expert = E_LOC * src + PIECES[src][cs[0]][0]
                for s in range(CAP):
                    start = table[0, SLOTS * expert + s]
                    for c in cs:
                        _, q, n = PIECES[src][c]
                        if n == 2:
                            row, parts = s, ((q, 0), (q + 1, 1))
                        elif s < 2 * HALF:
                            row, parts = s % HALF, ((q, s // HALF),)
                        elif _ends_pair(src, c):
                            row, parts = HALF, ((PIECES[src][c - 1][1], 0), (q, 1))
                        else:
                            continue
                        words = pieces[k, c, pl.ds(row, 1), :]
                        for tile, half in parts:
                            out_ref[pl.ds(start + SUBLANES * tile, 1), :] = _unpack(
                                words, half)
            elif op == "entered":
                wait_entered(pos)
            elif op == "ready":
                pl.semaphore_wait(ready_sem, 1)
            elif op == "flush":
                while flushed < len(sends) - args[0]:
                    sends[flushed].wait_send()
                    flushed += 1
        assert flushed == len(sends) and not (pending_rows or pending_w or pending_table)

        for tile in range(COL_TILES):
            out_ref[pl.ds(table[0, CAP] + SUBLANES * tile, 1), :] = jnp.zeros(
                (1, LANES), jnp.float32)

    schedules = _schedules()
    for pos in (D, A, B, Z):
        pl.when(me == pos)(lambda pos=pos: run(pos, schedules[pos]))


def pallas_dist_moe_cap_ep_n512_d256_e4_h512_kernel(
    x: jax.Array,
    router_W: jax.Array,
    route_idx: jax.Array,
    expert_W: jax.Array,
):
    del router_W
    max_sends = max(
        sum(step[0] == "send" for step in steps) for steps in _schedules().values())
    in_hbm = pl.BlockSpec(memory_space=pltpu.HBM)
    out = pl.pallas_call(
        _body,
        out_shape=jax.ShapeDtypeStruct((N_TOK * COL_TILES, LANES), jnp.float32),
        in_specs=[in_hbm, in_hbm, in_hbm],
        out_specs=pl.BlockSpec(memory_space=pltpu.VMEM),
        scratch_shapes=[
            pltpu.VMEM((N_TOK // LANES, LANES), jnp.int32),
            pltpu.VMEM((E_LOC * SLOTS, D_MODEL), jnp.float32),
            pltpu.VMEM((E_LOC, D_MODEL, D_OUT), jnp.float32),
            pltpu.VMEM((MAX_READS, D_MODEL, LANES), jnp.float32),
            pltpu.VMEM((N_DEV, MAX_PIECES, SLOTS, LANES), jnp.int32),
            pltpu.VMEM((1, N_EXP * SLOTS), jnp.int32),
            pltpu.SMEM((1, N_EXP * SLOTS), jnp.int32),
            pltpu.SemaphoreType.DMA,
            pltpu.SemaphoreType.DMA((E_LOC,)),
            pltpu.SemaphoreType.DMA((MAX_READS,)),
            pltpu.SemaphoreType.DMA,
            pltpu.SemaphoreType.DMA((max_sends + 1,)),
            pltpu.SemaphoreType.DMA(((N_DEV - 1) * MAX_PIECES,)),
            pltpu.SemaphoreType.REGULAR,
        ],
        compiler_params=pltpu.CompilerParams(
            collective_id=0,
            disable_bounds_checks=True,
            disable_semaphore_checks=True,
            flags={"XLA_TPU_FORCE_LP_LLO_SCHEDULER": True},
        ),
    )(route_idx.reshape(N_TOK // LANES, LANES), x, expert_W)
    out = out.reshape(N_TOK // SUBLANES, COL_TILES, SUBLANES, LANES)
    return out.transpose(0, 2, 1, 3).reshape(N_TOK, D_OUT)
```
